```python
import numpy as np

kernel_name = "dist_halo_stencil_i_m8192_n1024"

def setup_inputs():
    return {"x": np.random.randn(32768, 1024).astype(np.float32)}

def reference(x: np.ndarray) -> np.ndarray:
    out = np.empty_like(x)
    out[0] = x[0]
    out[-1] = x[-1]
    out[1:-1] = 0.25 * x[:-2] + 0.5 * x[1:-1] + 0.25 * x[2:]
    return out
```

```python
import jax
import jax.numpy as jnp
from jax import lax
from jax.experimental import pallas as pl
from jax.experimental.pallas import tpu as pltpu

N_DEV = 4
SUB = 8
LANE = 128
G, A, B = 2, 16, 32
COLS = G * B
STEPS = COLS - 2
AHEAD = 4

ICI_FIRST, ICI_LAST, RETURN = 16, 2, 8
ICI_PER_COL = COLS - 1 - ICI_FIRST
ICI_STRIPS = ICI_PER_COL + ICI_LAST

SMEM_HEAD = (10, A - 3, 3, None, 4)
SMEM_TAIL = (COLS - 1, ICI_LAST, 4, 52, 57)

LAST_READS = (
    (COLS - 2, 1, 8),
    (COLS - 2, 9, 7),
    (COLS - 1, 6, 5),
    (COLS - 1, 11, 3),
    (COLS - 1, 14, 2),
)
HALO_STEP = 36
CLEAR_UNROLL = 4


def _blend(above, here, below):
    return 0.25 * above + 0.5 * here + 0.25 * below


def _in_range(k, n):
    return jnp.logical_and(k >= 0, k < n)


def _strips(col, first, count):
    return (col // B, pl.ds(first, count), col % B)


def _stencil_kernel(
    x_hbm,
    y_ref,
    xb,
    halo,
    relay,
    smem_head,
    smem_tail,
    col_sems,
    last_sems,
    smem_sems,
    halo_send,
    halo_recv,
    leave_send,
    leave_recv,
    return_send,
    return_recv,
):
    n = x_hbm.shape[-1]

    def read(where, sem):
        return pltpu.make_async_copy(x_hbm.at[where], xb.at[where], sem)

    def start_column(col, first, count, sem):
        for c in range(n // LANE):
            where = _strips(col, first, count) + (slice(None), pl.ds(c * LANE, LANE))
            read(where, sem).start()

    def with_direct_strips(col, fn):
        first = _in_range(col - ICI_FIRST, ICI_PER_COL).astype(jnp.int32)
        count = jnp.where(col == SMEM_HEAD[0], A - SMEM_HEAD[2], A - first)
        for size in (A - SMEM_HEAD[2], A - 1, A):
            pl.when(count == size)(lambda: fn(first, size))

    def smem_detour(plan, buf, sem):
        where = _strips(*plan[:3])
        return (
            pltpu.make_async_copy(x_hbm.at[where], buf, sem),
            pltpu.make_async_copy(buf, xb.at[where], sem),
        )

    for col in range(AHEAD):
        start_column(col, 0, A, col_sems.at[col])
    head_load, head_forward = smem_detour(SMEM_HEAD, smem_head, smem_sems.at[0])
    tail_load, tail_forward = smem_detour(SMEM_TAIL, smem_tail, smem_sems.at[1])
    head_load.start()

    me = lax.axis_index("i")
    left = lax.rem(me + N_DEV - 1, N_DEV)
    right = lax.rem(me + 1, N_DEV)

    def remote(src, dst, send_sem, recv_sem, device):
        return pltpu.make_async_remote_copy(
            src, dst, send_sem, recv_sem,
            device_id=(device,), device_id_type=pl.DeviceIdType.MESH,
        )

    barrier = pltpu.get_barrier_semaphore()
    for neighbour in (left, right):
        pl.semaphore_signal(
            barrier, inc=1, device_id=(neighbour,), device_id_type=pl.DeviceIdType.MESH
        )

    first_row = x_hbm.at[0, 0, 0, pl.ds(0, 1)]
    last_row = x_hbm.at[G - 1, A - 1, B - 1, pl.ds(SUB - 1, 1)]
    halo_to_left = remote(first_row, halo.at[1], halo_send.at[0], halo_recv.at[1], left)
    halo_to_right = remote(last_row, halo.at[0], halo_send.at[1], halo_recv.at[0], right)

    def ici_strip(k):
        in_last = k >= ICI_PER_COL
        col = jnp.where(in_last, COLS - 1, ICI_FIRST + k)
        return _strips(col, jnp.where(in_last, k - ICI_PER_COL, 0), 1)

    def leave(k):
        device = jnp.where(k % 2 == 0, left, right)
        slot = relay.at[pl.ds(k, 1)]
        return remote(x_hbm.at[ici_strip(k)], slot, leave_send, leave_recv.at[k], device)

    def send_back(k):
        device = jnp.where(k % 2 == 0, right, left)
        slot = relay.at[pl.ds(k, 1)]
        return remote(slot, xb.at[ici_strip(k)], return_send, return_recv.at[k], device)

    sub = lax.broadcasted_iota(jnp.int32, (SUB, n), 0)

    def lanes(b):
        start = b * n if isinstance(b, int) else pl.multiple_of(b * n, n)
        return pl.ds(start, n)

    def clear(b):
        for g in range(G):
            for r in (0, A * SUB):
                y_ref[g, pl.ds(r, SUB), lanes(b)] = jnp.zeros((SUB, n), y_ref.dtype)

    def strip(g, a, b, b_prev):
        prev, cur = xb[g, a, b_prev], xb[g, a, b]
        z = _blend(
            pltpu.roll(jnp.where(sub >= SUB - 2, prev, cur), 2, 0),
            pltpu.roll(jnp.where(sub >= SUB - 1, prev, cur), 1, 0),
            cur,
        )
        pltpu.store(y_ref.at[g, pl.ds(a * SUB, SUB), lanes(b)], z, mask=sub >= 1)
        pltpu.store(y_ref.at[g, pl.ds((a + 1) * SUB, SUB), lanes(b_prev)], z, mask=sub < 1)

    def row(g, a, b, s):
        return xb[g, a, b, pl.ds(s, 1), :]

    def seam(g, a):
        second_last, last = row(g, a, B - 1, SUB - 2), row(g, a, B - 1, SUB - 1)
        if (g, a) == (G - 1, A - 1):
            out = jnp.where(me == N_DEV - 1, last, _blend(second_last, last, halo[1]))
        else:
            g_next, a_next = (g, a + 1) if a + 1 < A else (g + 1, 0)
            first, second = row(g_next, a_next, 0, 0), row(g_next, a_next, 0, 1)
            out = _blend(second_last, last, first)
            y_ref[g_next, pl.ds(a_next * SUB + 1, 1), lanes(0)] = _blend(last, first, second)
        y_ref[g, pl.ds((a + 1) * SUB, 1), lanes(B - 1)] = out

    for b in range(CLEAR_UNROLL):
        clear(b)
    pl.loop(CLEAR_UNROLL, B)(clear)

    @pl.loop(0, STEPS)
    def _(j):
        sem = col_sems.at[j % AHEAD]
        with_direct_strips(j, lambda *r: read(_strips(j, *r), sem).wait())

        @pl.when(j == 0)
        def _():
            pl.semaphore_wait(barrier, 2)
            halo_to_left.start()
            halo_to_right.start()

        pl.when(j < ICI_STRIPS)(lambda: leave(j).start())

        @pl.when(j + AHEAD < STEPS)
        def _():
            with_direct_strips(j + AHEAD, lambda *r: start_column(j + AHEAD, *r, sem))

        for col in (COLS - 2, COLS - 1):

            @pl.when(j + AHEAD == col)
            def _():
                for t, piece in enumerate(LAST_READS):
                    if piece[0] == col:
                        read(_strips(*piece), last_sems.at[t]).start()

        @pl.when(_in_range(j - RETURN, ICI_STRIPS))
        def _():
            leave(j - RETURN).wait_recv()
            send_back(j - RETURN).start()

        pl.when(j >= ICI_FIRST)(lambda: send_back(j - ICI_FIRST).wait_recv())

        @pl.when(j == SMEM_HEAD[4])
        def _():
            head_load.wait()
            head_forward.start()

        pl.when(j == SMEM_HEAD[0])(head_forward.wait)
        pl.when(j == SMEM_TAIL[3])(tail_load.start)

        @pl.when(j == SMEM_TAIL[4])
        def _():
            tail_load.wait()
            tail_forward.start()

        b = j % B
        for a in range(A):
            strip(j // B, a, b, jnp.maximum(b - 1, 0))

        for g in range(G - 1):

            @pl.when(j == (g + 1) * B)
            def _():
                for a in range(A):
                    seam(g, a)

        @pl.when(j == HALO_STEP)
        def _():
            halo_to_left.wait()
            halo_to_right.wait()
            first = row(0, 0, 0, 0)
            out = jnp.where(me == 0, first, _blend(halo[0], first, row(0, 0, 0, 1)))
            y_ref[0, pl.ds(1, 1), lanes(0)] = out

    def finish(col, first, count):
        for a in range(first, first + count):
            strip(G - 1, a, col % B, col % B - 1)
            if col == COLS - 1:
                seam(G - 1, a)

    def finish_reads(col):
        for t, piece in enumerate(LAST_READS):
            if piece[0] == col:
                read(_strips(*piece), last_sems.at[t]).wait()
                finish(*piece)

    send_back(ICI_PER_COL - 1).wait_recv()
    finish(COLS - 2, 0, 1)
    finish_reads(COLS - 2)
    for k in range(ICI_PER_COL, ICI_STRIPS):
        send_back(k).wait_recv()
    finish(COLS - 1, 0, ICI_LAST)
    pltpu.make_async_copy(relay, relay, leave_send).wait()
    pltpu.make_async_copy(relay, relay, return_send).wait()
    tail_forward.wait()
    finish(*SMEM_TAIL[:3])
    finish_reads(COLS - 1)


def pallas_dist_halo_stencil_i_m8192_n1024_kernel(
    x: jax.Array,
):
    m, n = x.shape
    assert m == G * A * B * SUB and n % LANE == 0, x.shape
    dma = pltpu.SemaphoreType.DMA
    y = pl.pallas_call(
        _stencil_kernel,
        out_shape=jax.ShapeDtypeStruct((G, (A + 1) * SUB, B * n), x.dtype),
        in_specs=[pl.BlockSpec(memory_space=pl.ANY)],
        out_specs=pl.BlockSpec(memory_space=pltpu.VMEM),
        scratch_shapes=[
            pltpu.VMEM((G, A, B, SUB, n), x.dtype),
            pltpu.VMEM((2, 1, n), x.dtype),
            pltpu.VMEM((ICI_STRIPS, SUB, n), x.dtype),
            pltpu.SMEM((SMEM_HEAD[2], SUB, n), x.dtype),
            pltpu.SMEM((SMEM_TAIL[2], SUB, n), x.dtype),
            dma((AHEAD,)),
            dma((len(LAST_READS),)),
            dma((2,)),
            dma((2,)),
            dma((2,)),
            dma,
            dma((ICI_STRIPS,)),
            dma,
            dma((ICI_STRIPS,)),
        ],
        compiler_params=pltpu.CompilerParams(
            collective_id=0,
            vmem_limit_bytes=72 * 2**20,
            disable_bounds_checks=True,
            disable_semaphore_checks=True,
        ),
    )(x.reshape(G, A, B, SUB, n))
    y = y[:, 1 : A * SUB + 1].reshape(G, A, SUB, B, n)
    return y.transpose(0, 1, 3, 2, 4).reshape(m, n)
```

```python
import jax
import jax.numpy as jnp
from jax import lax
from jax.experimental import pallas as pl
from jax.experimental.pallas import tpu as pltpu

N_DEV = 4
SUB = 8
LANE = 128
G, A, B = 2, 16, 32
COLS = G * B
STEPS = COLS - 2
AHEAD = 4

ICI_FIRST, ICI_LAST, RETURN = 16, 2, 8
ICI_PER_COL = COLS - 1 - ICI_FIRST
ICI_STRIPS = ICI_PER_COL + ICI_LAST

SMEM_HEAD = (10, A - 3, 3, None, 4)
SMEM_TAIL = (COLS - 1, ICI_LAST, 4, 52, 57)

LAST_READS = (
    (COLS - 2, 1, 8),
    (COLS - 2, 9, 7),
    (COLS - 1, 6, 5),
    (COLS - 1, 11, 3),
    (COLS - 1, 14, 2),
)
HALO_STEP = 36
CLEAR_UNROLL = 4


def _blend(above, here, below):
    return 0.25 * above + 0.5 * here + 0.25 * below


def _in_range(k, n):
    return jnp.logical_and(k >= 0, k < n)


def _strips(col, first, count):
    return (col // B, pl.ds(first, count), col % B)


def _stencil_kernel(
    x_hbm,
    y_ref,
    xb,
    halo,
    relay,
    smem_head,
    smem_tail,
    col_sems,
    last_sems,
    smem_sems,
    halo_send,
    halo_recv,
    leave_send,
    leave_recv,
    return_send,
    return_recv,
):
    n = x_hbm.shape[-1]

    def read(where, sem):
        return pltpu.make_async_copy(x_hbm.at[where], xb.at[where], sem)

    def start_column(col, first, count, sem):
        for c in range(n // LANE):
            where = _strips(col, first, count) + (slice(None), pl.ds(c * LANE, LANE))
            read(where, sem).start()

    def with_direct_strips(col, fn):
        first = _in_range(col - ICI_FIRST, ICI_PER_COL).astype(jnp.int32)
        count = jnp.where(col == SMEM_HEAD[0], A - SMEM_HEAD[2], A - first)
        for size in (A - SMEM_HEAD[2], A - 1, A):
            pl.when(count == size)(lambda: fn(first, size))

    def smem_detour(plan, buf, sem):
        where = _strips(*plan[:3])
        return (
            pltpu.make_async_copy(x_hbm.at[where], buf, sem),
            pltpu.make_async_copy(buf, xb.at[where], sem),
        )

    for col in range(AHEAD):
        start_column(col, 0, A, col_sems.at[col])
    head_load, head_forward = smem_detour(SMEM_HEAD, smem_head, smem_sems.at[0])
    tail_load, tail_forward = smem_detour(SMEM_TAIL, smem_tail, smem_sems.at[1])
    head_load.start()

    me = lax.axis_index("i")
    left = lax.rem(me + N_DEV - 1, N_DEV)
    right = lax.rem(me + 1, N_DEV)

    def remote(src, dst, send_sem, recv_sem, device):
        return pltpu.make_async_remote_copy(
            src, dst, send_sem, recv_sem,
            device_id=(device,), device_id_type=pl.DeviceIdType.MESH,
        )

    barrier = pltpu.get_barrier_semaphore()
    for neighbour in (left, right):
        pl.semaphore_signal(
            barrier, inc=1, device_id=(neighbour,), device_id_type=pl.DeviceIdType.MESH
        )

    first_row = x_hbm.at[0, 0, 0, pl.ds(0, 1)]
    last_row = x_hbm.at[G - 1, A - 1, B - 1, pl.ds(SUB - 1, 1)]
    halo_to_left = remote(first_row, halo.at[1], halo_send.at[0], halo_recv.at[1], left)
    halo_to_right = remote(last_row, halo.at[0], halo_send.at[1], halo_recv.at[0], right)

    def ici_strip(k):
        in_last = k >= ICI_PER_COL
        col = jnp.where(in_last, COLS - 1, ICI_FIRST + k)
        return _strips(col, jnp.where(in_last, k - ICI_PER_COL, 0), 1)

    def leave(k):
        device = jnp.where(k % 2 == 0, left, right)
        slot = relay.at[pl.ds(k, 1)]
        return remote(x_hbm.at[ici_strip(k)], slot, leave_send.at[k], leave_recv.at[k], device)

    def send_back(k):
        device = jnp.where(k % 2 == 0, right, left)
        slot = relay.at[pl.ds(k, 1)]
        return remote(slot, xb.at[ici_strip(k)], return_send.at[k], return_recv.at[k], device)

    sub = lax.broadcasted_iota(jnp.int32, (SUB, n), 0)

    def lanes(b):
        start = b * n if isinstance(b, int) else pl.multiple_of(b * n, n)
        return pl.ds(start, n)

    def clear(b):
        for g in range(G):
            for r in (0, A * SUB):
                y_ref[g, pl.ds(r, SUB), lanes(b)] = jnp.zeros((SUB, n), y_ref.dtype)

    def strip(g, a, b, b_prev):
        prev, cur = xb[g, a, b_prev], xb[g, a, b]
        z = _blend(
            pltpu.roll(jnp.where(sub >= SUB - 2, prev, cur), 2, 0),
            pltpu.roll(jnp.where(sub >= SUB - 1, prev, cur), 1, 0),
            cur,
        )
        pltpu.store(y_ref.at[g, pl.ds(a * SUB, SUB), lanes(b)], z, mask=sub >= 1)
        pltpu.store(y_ref.at[g, pl.ds((a + 1) * SUB, SUB), lanes(b_prev)], z, mask=sub < 1)

    def row(g, a, b, s):
        return xb[g, a, b, pl.ds(s, 1), :]

    def seam(g, a):
        second_last, last = row(g, a, B - 1, SUB - 2), row(g, a, B - 1, SUB - 1)
        if (g, a) == (G - 1, A - 1):
            out = jnp.where(me == N_DEV - 1, last, _blend(second_last, last, halo[1]))
        else:
            g_next, a_next = (g, a + 1) if a + 1 < A else (g + 1, 0)
            first, second = row(g_next, a_next, 0, 0), row(g_next, a_next, 0, 1)
            out = _blend(second_last, last, first)
            y_ref[g_next, pl.ds(a_next * SUB + 1, 1), lanes(0)] = _blend(last, first, second)
        y_ref[g, pl.ds((a + 1) * SUB, 1), lanes(B - 1)] = out

    for b in range(CLEAR_UNROLL):
        clear(b)
    pl.loop(CLEAR_UNROLL, B)(clear)

    @pl.loop(0, STEPS)
    def _(j):
        sem = col_sems.at[j % AHEAD]
        with_direct_strips(j, lambda *r: read(_strips(j, *r), sem).wait())

        @pl.when(j == 0)
        def _():
            pl.semaphore_wait(barrier, 2)
            halo_to_left.start()
            halo_to_right.start()

        pl.when(j < ICI_STRIPS)(lambda: leave(j).start())

        @pl.when(j + AHEAD < STEPS)
        def _():
            with_direct_strips(j + AHEAD, lambda *r: start_column(j + AHEAD, *r, sem))

        for col in (COLS - 2, COLS - 1):

            @pl.when(j + AHEAD == col)
            def _():
                for t, piece in enumerate(LAST_READS):
                    if piece[0] == col:
                        read(_strips(*piece), last_sems.at[t]).start()

        @pl.when(_in_range(j - RETURN, ICI_STRIPS))
        def _():
            leave(j - RETURN).wait()
            send_back(j - RETURN).start()

        pl.when(j >= ICI_FIRST)(lambda: send_back(j - ICI_FIRST).wait())

        @pl.when(j == SMEM_HEAD[4])
        def _():
            head_load.wait()
            head_forward.start()

        pl.when(j == SMEM_HEAD[0])(head_forward.wait)
        pl.when(j == SMEM_TAIL[3])(tail_load.start)

        @pl.when(j == SMEM_TAIL[4])
        def _():
            tail_load.wait()
            tail_forward.start()

        b = j % B
        for a in range(A):
            strip(j // B, a, b, jnp.maximum(b - 1, 0))

        for g in range(G - 1):

            @pl.when(j == (g + 1) * B)
            def _():
                for a in range(A):
                    seam(g, a)

        @pl.when(j == HALO_STEP)
        def _():
            halo_to_left.wait()
            halo_to_right.wait()
            first = row(0, 0, 0, 0)
            out = jnp.where(me == 0, first, _blend(halo[0], first, row(0, 0, 0, 1)))
            y_ref[0, pl.ds(1, 1), lanes(0)] = out

    def finish(col, first, count):
        for a in range(first, first + count):
            strip(G - 1, a, col % B, col % B - 1)
            if col == COLS - 1:
                seam(G - 1, a)

    def finish_reads(col):
        for t, piece in enumerate(LAST_READS):
            if piece[0] == col:
                read(_strips(*piece), last_sems.at[t]).wait()
                finish(*piece)

    send_back(ICI_PER_COL - 1).wait()
    finish(COLS - 2, 0, 1)
    finish_reads(COLS - 2)
    for k in range(ICI_PER_COL, ICI_STRIPS):
        send_back(k).wait()
    finish(COLS - 1, 0, ICI_LAST)
    tail_forward.wait()
    finish(*SMEM_TAIL[:3])
    finish_reads(COLS - 1)


def pallas_dist_halo_stencil_i_m8192_n1024_kernel(
    x: jax.Array,
):
    m, n = x.shape
    assert m == G * A * B * SUB and n % LANE == 0, x.shape
    dma = pltpu.SemaphoreType.DMA
    y = pl.pallas_call(
        _stencil_kernel,
        out_shape=jax.ShapeDtypeStruct((G, (A + 1) * SUB, B * n), x.dtype),
        in_specs=[pl.BlockSpec(memory_space=pl.ANY)],
        out_specs=pl.BlockSpec(memory_space=pltpu.VMEM),
        scratch_shapes=[
            pltpu.VMEM((G, A, B, SUB, n), x.dtype),
            pltpu.VMEM((2, 1, n), x.dtype),
            pltpu.VMEM((ICI_STRIPS, SUB, n), x.dtype),
            pltpu.SMEM((SMEM_HEAD[2], SUB, n), x.dtype),
            pltpu.SMEM((SMEM_TAIL[2], SUB, n), x.dtype),
            dma((AHEAD,)),
            dma((len(LAST_READS),)),
            dma((2,)),
            dma((2,)),
            dma((2,)),
            dma((ICI_STRIPS,)),
            dma((ICI_STRIPS,)),
            dma((ICI_STRIPS,)),
            dma((ICI_STRIPS,)),
        ],
        compiler_params=pltpu.CompilerParams(
            collective_id=0,
            vmem_limit_bytes=72 * 2**20,
            disable_bounds_checks=True,
            disable_semaphore_checks=True,
        ),
    )(x.reshape(G, A, B, SUB, n))
    y = y[:, 1 : A * SUB + 1].reshape(G, A, SUB, B, n)
    return y.transpose(0, 1, 3, 2, 4).reshape(m, n)
```
